```python
import numpy as np

kernel_name = "dist_f_of_ar_i_m4096_n1024"

def setup_inputs():
    t = np.random.randn(16384, 1024).astype(np.float32)
    return {"t": t}

def reference(t: np.ndarray) -> np.ndarray:
    s = t.reshape(4, 4096, 1024).sum(axis=0)
    r = np.maximum(s, 0.0)
    return np.tanh(s) * s * s + r * r * r
```

```python
import jax
import jax.numpy as jnp
from jax import lax
from jax.experimental import pallas as pl
from jax.experimental.pallas import tpu as pltpu

M = 4096
N = 1024
E = 512
HR = 16
HW = 768
HO = E - HR
BLK = 16
NRAMP = 2

S1A = (16, 32, 64, 128, 256)
S1B = (240, 256)
S2 = (256, 256)
S4A = (512,)
S4B = (448, 48, 16)

ROOT, LATE = 0, 2
MESH = pl.DeviceIdType.MESH
BF16, F32 = jnp.bfloat16, jnp.float32


def _chunks(sizes, o=0):
    out = []
    for s in sizes:
        out.append((o, s))
        o += s
    return out


C1 = _chunks(S1A) + _chunks(S1B, E)
C2, C4A, C4B = _chunks(S2), _chunks(S4A), _chunks(S4B)

_REM, _LOC = {}, {}
for _h in range(2):
    for _key in (
        [("1", _j) for _j in range(len(C1))]
        + [("hL", 0), ("hR", 0), ("m", 0), ("x", 0)]
        + [("2", _j) for _j in range(len(C2))]
        + [("3", _j) for _j in range(len(C2))]
        + [("4a", _j) for _j in range(len(C4A))]
        + [("4b", _j) for _j in range(len(C4B))]
    ):
        _REM[(_h,) + _key] = len(_REM)
    for _key in [("ld", _j) for _j in range(len(C1))] + [("ldh", 0), ("ldm", 0), ("ldk", 2), ("ldk", 3)]:
        _LOC[(_h,) + _key] = len(_LOC)


def _rows(o, s, fn):
    n = s // BLK
    if n == 1:
        fn(o, BLK)
    else:
        def step(i, c):
            fn(pl.multiple_of(o + i * BLK, BLK), BLK)
            return c
        lax.fori_loop(0, n, step, 0)


def _body(t_ref, oa_ref, ob_ref, xs, xk, send1, recv1, send2, recv2, gath, xtra,
          ssem, rsem, lsem, hs):
    outs = (oa_ref, ob_ref)
    bar = pltpu.get_barrier_semaphore()

    def sig(sem, dev):
        pl.semaphore_signal(sem, inc=1, device_id=(dev,), device_id_type=MESH)

    def program(me):
        x = me >> 1
        y = (me ^ x) & 1
        ynbr, xnbr = me ^ 1, 3 - me
        c1, c2 = (y, x), (x, y)
        p1, p2 = (ynbr, xnbr), (xnbr, ynbr)
        off = [[(c1[h] if role >= 2 else 1 - c1[h]) * 2 * E
                + (c2[h] if role in (1, 3) else 1 - c2[h]) * E
                for role in range(4)] for h in range(2)]
        e = {1: 0, 3: 1}.get(me)
        horder = (0, 1) if e is None else (e, 1 - e)

        def ld(key, h, o, s):
            g = h * (M // 2) + off[h][o // E] + o % E
            return pltpu.make_async_copy(t_ref.at[pl.ds(g, s)], xs.at[h, pl.ds(o, s)],
                                         lsem.at[_LOC[(h,) + key]])

        def ld1(h, j): return ld(("ld", j), h, *C1[j])
        def ldh(h): return ld(("ldh", 0), h, HO, HR)
        def ldm(h): return ld(("ldm", 0), h, E + HO, HR)

        def ldk(h, role):
            return pltpu.make_async_copy(t_ref.at[pl.ds(h * (M // 2) + off[h][role], E)],
                                         xk.at[h, role - 2], lsem.at[_LOC[(h, "ldk", role)]])

        def rcopy(key, src, dst, dev):
            i = _REM[key]
            return pltpu.make_async_remote_copy(
                src_ref=src, dst_ref=dst, send_sem=ssem.at[i], recv_sem=rsem.at[i],
                device_id=(dev,), device_id_type=MESH)

        hrows, mrows = pl.ds(HO, HR), pl.ds(E + HO, HR)
        lcols, rcols = pl.ds(0, HW), pl.ds(HW, N - HW)

        def r1(h, j):
            r = pl.ds(*C1[j])
            return rcopy((h, "1", j), send1.at[h, r], recv1.at[h, r], p1[h])

        def rhl(h): return rcopy((h, "hL", 0), send1.at[h, hrows, lcols], recv1.at[h, hrows, lcols], p1[h])
        def rhr(h): return rcopy((h, "hR", 0), send1.at[h, hrows, rcols], recv1.at[h, hrows, rcols], p1[h])
        def rx(h): return rcopy((h, "x", 0), send1.at[h, hrows, lcols], xtra.at[h], LATE)
        def rm(h): return rcopy((h, "m", 0), send1.at[h, mrows], recv1.at[h, mrows], p1[h])

        def r2(h, j):
            r = pl.ds(*C2[j])
            return rcopy((h, "2", j), send2.at[h, r], recv2.at[h, r], p2[h])

        def r3(h, j):
            r = pl.ds(*C2[j])
            return rcopy((h, "3", j), gath.at[h, 3, r], gath.at[h, 2, r], p2[h])

        def r4a(h, j):
            r = pl.ds(*C4A[j])
            return rcopy((h, "4a", j), gath.at[h, 3, r], gath.at[h, 1, r], p1[h])

        def r4b(h, j):
            r = pl.ds(*C4B[j])
            return rcopy((h, "4b", j), gath.at[h, 2, r], gath.at[h, 0, r], p1[h])

        sent = []

        def go(cp):
            cp.start()
            sent.append(cp)

        def cvt(h, o, s):
            def f(r, b):
                send1[h, pl.ds(r, b), :] = xs[h, pl.ds(r, b), :].astype(BF16)
            _rows(o, s, f)

        def prep(h, j):
            ld1(h, j).wait()
            cvt(h, *C1[j])

        def ld_rest(j0):
            for j in range(j0, len(S1A)):
                for h in horder:
                    ld1(h, j).start()
            for h in horder:
                ldh(h).start()
            for j in range(len(S1A), len(C1)):
                for h in horder:
                    ld1(h, j).start()
            for h in horder:
                ldm(h).start()
            for role in (2, 3):
                for h in range(2):
                    ldk(h, role).start()

        if me == ROOT:
            sig(bar, 1)
            sig(bar, 3)
            ld_rest(0)
            for j in range(NRAMP):
                for h in range(2):
                    prep(h, j)
            for h in range(2):
                pl.semaphore_wait(hs.at[h], 1)
                for j in range(NRAMP):
                    go(r1(h, j))
        elif me == LATE:
            ld1(0, 0).start()
            ld1(1, 0).start()
            pl.semaphore_wait(bar, 2)
            sig(hs.at[0], 3)
            sig(hs.at[1], 1)
            ld_rest(1)
            for j in range(NRAMP):
                for h in range(2):
                    prep(h, j)
                    go(r1(h, j))
        else:
            l = 1 - e
            sig(bar, LATE)
            ld1(e, 0).start()
            pl.semaphore_wait(bar, 1)
            sig(hs.at[e], ROOT)
            ld1(l, 0).start()
            ld_rest(1)
            for j in range(NRAMP):
                prep(e, j)
                go(r1(e, j))
                prep(l, j)
            pl.semaphore_wait(hs.at[l], 1)
            for j in range(NRAMP):
                go(r1(l, j))

        for j in range(NRAMP, len(S1A)):
            for h in horder:
                prep(h, j)
                go(r1(h, j))
        for h in horder:
            ldh(h).wait()
            cvt(h, HO, HR)
            go(rx(h) if e == h else rhl(h))
            go(rhr(h))
        for j in range(len(S1A), len(C1)):
            for h in horder:
                prep(h, j)
                go(r1(h, j))
        if me != LATE:
            for h in horder:
                ldm(h).wait()
                cvt(h, E + HO, HR)
                go(rm(h))

        waited = set()

        def wait1(h, lo, hi):
            for j, (o, s) in enumerate(C1):
                if o < hi and o + s > lo and (h, j) not in waited:
                    waited.add((h, j))
                    r1(h, j).wait_recv()
            if lo < E and hi > HO and (h, "h") not in waited:
                waited.add((h, "h"))
                if me != ROOT:
                    rhl(h).wait_recv()
                rhr(h).wait_recv()
            if hi > E + HO and (h, "m") not in waited:
                waited.add((h, "m"))
                rm(h).wait_recv()

        for j, (o, s) in enumerate(C2):
            for h in range(2):
                if j == 0:
                    ldk(h, 2).wait()
                wait1(h, o, o + s)

                def add(r, b, h=h):
                    send2[h, pl.ds(r, b), :] = (
                        xk[h, 0, pl.ds(r, b), :] + recv1[h, pl.ds(r, b), :].astype(F32)).astype(BF16)

                if me == ROOT and o + s == E:
                    _rows(o, s - HR, add)
                    send2[h, hrows, lcols] = xk[h, 0, hrows, lcols].astype(BF16)
                    send2[h, hrows, rcols] = (
                        xk[h, 0, hrows, rcols] + recv1[h, hrows, rcols].astype(F32)).astype(BF16)
                else:
                    _rows(o, s, add)
                go(r2(h, j))
            if j == 0 and me == LATE:
                for h in range(2):
                    ldm(h).wait()
                    rx(h).wait_recv()
                    send1[h, mrows, lcols] = (xs[h, mrows, lcols] + xtra[h].astype(F32)).astype(BF16)
                    send1[h, mrows, rcols] = xs[h, mrows, rcols].astype(BF16)
                    go(rm(h))

        def pre(h, o, s):
            wait1(h, E + o, E + o + s)

            def f(r, b):
                xk[h, 1, pl.ds(r, b), :] = (
                    xk[h, 1, pl.ds(r, b), :] + recv1[h, pl.ds(E + r, b), :].astype(F32))
            _rows(o, s, f)

        for h in range(2):
            ldk(h, 3).wait()
            pre(h, 0, HO)

        for j, (o, s) in enumerate(C2):
            if j == len(C2) - 1:
                for h in range(2):
                    pre(h, HO, HR)
            for h in range(2):
                r2(h, j).wait_recv()

                def fin(r, b, h=h):
                    sv = xk[h, 1, pl.ds(r, b), :] + recv2[h, pl.ds(r, b), :].astype(F32)
                    rl = jnp.maximum(sv, 0.0)
                    v = jnp.tanh(sv) * sv * sv + rl * rl * rl
                    outs[h][pl.ds(pl.multiple_of(off[h][3] + r, BLK), b), :] = v
                    gath[h, 3, pl.ds(r, b), :] = v.astype(BF16)

                _rows(o, s, fin)
                go(r3(h, j))
        for j in range(len(C4A)):
            for h in range(2):
                go(r4a(h, j))

        def up(h, role, o, s):
            def f(r, b):
                outs[h][pl.ds(pl.multiple_of(off[h][role] + r, BLK), b), :] = (
                    gath[h, role, pl.ds(r, b), :].astype(F32))
            _rows(o, s, f)

        n_early = None
        started = set()
        for j, (o, s) in enumerate(C2):
            for h in range(2):
                r3(h, j).wait_recv()
                for jj, (oo, ss) in enumerate(C4B):
                    if oo + ss <= o + s and (h, jj) not in started:
                        if n_early is None:
                            n_early = len(sent)
                        started.add((h, jj))
                        go(r4b(h, jj))
            for h in range(2):
                up(h, 2, o, s)

        for j, (o, s) in enumerate(C4A):
            for h in range(2):
                r4a(h, j).wait_recv()
                up(h, 1, o, s)
        for j, (o, s) in enumerate(C4B):
            if j == len(C4B) - 1:
                for cp in sent[:n_early]:
                    cp.wait_send()
            for h in range(2):
                r4b(h, j).wait_recv()
                up(h, 0, o, s)
        for cp in sent[n_early:]:
            cp.wait_send()

    me_dyn = lax.axis_index("i")
    for d in range(4):
        pl.when(me_dyn == d)(lambda d=d: program(d))


def pallas_dist_f_of_ar_i_m4096_n1024_kernel(
t: jax.Array,
):
    oa, ob = pl.pallas_call(
        _body,
        out_shape=[jax.ShapeDtypeStruct((M // 2, N), F32)] * 2,
        in_specs=[pl.BlockSpec(memory_space=pl.ANY)],
        out_specs=[pl.BlockSpec(memory_space=pltpu.VMEM)] * 2,
        scratch_shapes=[
            pltpu.VMEM((2, 2 * E, N), F32),
            pltpu.VMEM((2, 2, E, N), F32),
            pltpu.VMEM((2, 2 * E, N), BF16),
            pltpu.VMEM((2, 2 * E, N), BF16),
            pltpu.VMEM((2, E, N), BF16),
            pltpu.VMEM((2, E, N), BF16),
            pltpu.VMEM((2, 4, E, N), BF16),
            pltpu.VMEM((2, HR, HW), BF16),
            pltpu.SemaphoreType.DMA((len(_REM),)),
            pltpu.SemaphoreType.DMA((len(_REM),)),
            pltpu.SemaphoreType.DMA((len(_LOC),)),
            pltpu.SemaphoreType.REGULAR((2,)),
        ],
        compiler_params=pltpu.CompilerParams(
            collective_id=0,
            vmem_limit_bytes=64 * 1024 * 1024,
            disable_semaphore_checks=True,
        ),
    )(t)
    return jnp.concatenate([oa, ob], axis=0)
```
